```python
import numpy as np

kernel_name = "dist_rope_attn_qseq_b2_sq128_d512_hq4_dh64"

def setup_inputs():
    x = np.random.randn(2, 512, 512).astype(np.float32)
    Wq = np.random.randn(512, 256).astype(np.float32) * 0.02
    Wk = np.random.randn(512, 256).astype(np.float32) * 0.02
    Wv = np.random.randn(512, 256).astype(np.float32) * 0.02
    Wo = np.random.randn(256, 512).astype(np.float32) * 0.02
    return {"x": x, "Wq": Wq, "Wk": Wk, "Wv": Wv, "Wo": Wo}

def reference(x, Wq, Wk, Wv, Wo):
    B, Sq, Hq, Dh = 2, 512, 4, 64
    inv = 1.0 / (10000.0 ** (np.arange(0, Dh, 2) / Dh))
    pos = np.arange(Sq)[:, None] * inv[None, :]
    cos = np.repeat(np.cos(pos), 2, axis=-1).astype(np.float32)
    sin = np.repeat(np.sin(pos), 2, axis=-1).astype(np.float32)
    def rot(t):
        t2 = t.reshape(B, Sq, Hq, Dh // 2, 2)
        t_r = np.stack([-t2[..., 1], t2[..., 0]], axis=-1).reshape(B, Sq, Hq, Dh)
        return t * cos[None, :, None, :] + t_r * sin[None, :, None, :]
    Q = rot((x @ Wq).reshape(B, Sq, Hq, Dh))
    K = rot((x @ Wk).reshape(B, Sq, Hq, Dh))
    V = (x @ Wv).reshape(B, Sq, Hq, Dh)
    s = np.einsum('bihd,bjhd->bhij', Q, K).astype(np.float32) * 0.125
    s_max = s.max(axis=-1, keepdims=True)
    w = np.exp(s - s_max)
    w = w / w.sum(axis=-1, keepdims=True)
    ctx = np.einsum('bhij,bjhd->bihd', w, V).reshape(B, Sq, Hq * Dh)
    return ctx @ Wo
```

```python
import functools
import numpy as np
import jax
import jax.numpy as jnp
from jax import lax
from jax.experimental import pallas as pl
from jax.experimental.pallas import tpu as pltpu

SQ = 128
DM = 512
HD = 256
DH = 64


def _rope_tables():
    inv = 1.0 / (10000.0 ** (np.arange(0, DH, 2) / DH))
    pos = np.arange(4 * SQ)[:, None] * inv[None, :]
    cos = np.repeat(np.cos(pos), 2, axis=-1).astype(np.float32)
    sin = np.repeat(np.sin(pos), 2, axis=-1).astype(np.float32)
    sgn = np.where(np.arange(DH) % 2 == 0, -1.0, 1.0).astype(np.float32)
    sin = sin * sgn[None, :]
    t = np.concatenate([cos, sin], axis=-1).reshape(4, SQ, 128)
    out = np.stack([np.stack([t[i], t[i ^ 1], t[3 - i]]) for i in range(4)])
    return np.ascontiguousarray(out)


_TAB = _rope_tables()
NCH = 2
CR = SQ // NCH


def pallas_dist_rope_attn_qseq_b2_sq128_d512_hq4_dh64_kernel(x, Wq, Wk, Wv, Wo):
    f32, bf16 = jnp.float32, jnp.bfloat16
    MESH = pl.DeviceIdType.MESH
    NT = (((1,), (1,)), ((), ()))

    def body(x_hbm, wq_hbm, wk_hbm, wv_hbm, wo_hbm, tab_hbm, out_ref,
             xf, xs, xo, xa, xb, wf, wof, wq_b, wkv_b, wo_b, tab, kv, qm, ctxs, ctxr,
             lsem, ssem, rsem):
        me = lax.axis_index("i")
        A = me ^ 1
        B = 3 - me
        b = ((me + 1) >> 1) & 1

        bar = pltpu.get_barrier_semaphore()
        pl.semaphore_signal(bar, inc=1, device_id=(A,), device_id_type=MESH)
        pl.semaphore_signal(bar, inc=1, device_id=(B,), device_id_type=MESH)

        def rows(c):
            return pl.ds(c * CR, CR)
        ld_xo = [pltpu.make_async_copy(x_hbm.at[b, rows(c)], xf.at[1, rows(c)], lsem.at[c]) for c in range(NCH)]
        ld_xs = [pltpu.make_async_copy(x_hbm.at[1 - b, rows(c)], xf.at[0, rows(c)], lsem.at[NCH + c]) for c in range(NCH)]
        o = 2 * NCH
        ld_wk = pltpu.make_async_copy(wk_hbm, wf.at[1], lsem.at[o])
        ld_wv = pltpu.make_async_copy(wv_hbm, wf.at[2], lsem.at[o + 1])
        ld_wq = pltpu.make_async_copy(wq_hbm, wf.at[0], lsem.at[o + 2])
        ld_wo = pltpu.make_async_copy(wo_hbm, wof, lsem.at[o + 3])
        ld_tab = pltpu.make_async_copy(tab_hbm.at[me], tab, lsem.at[o + 4])
        for c in range(NCH):
            ld_xo[c].start()
            ld_xs[c].start()
        ld_wk.start(); ld_wv.start(); ld_tab.start(); ld_wq.start(); ld_wo.start()

        def rcopy(src, dst, si, ri, dev):
            return pltpu.make_async_remote_copy(src, dst, ssem.at[si], rsem.at[ri], device_id=(dev,), device_id_type=MESH)
        snd_xa = [rcopy(xs.at[rows(c)], xa.at[rows(c)], c, c, A) for c in range(NCH)]
        snd_xb = [rcopy(xo.at[rows(c)], xb.at[rows(c)], NCH + c, NCH + c, B) for c in range(NCH)]
        o = 2 * NCH
        fwd = [[rcopy(kv.at[p, :, pl.ds(SQ + c * CR, CR)], kv.at[p, :, pl.ds(3 * SQ + c * CR, CR)],
                      o + 2 * c + p, o + 2 * c + p, B) for p in range(2)] for c in range(NCH)]
        o = 2 * NCH + 2 * NCH
        ret = [rcopy(ctxs.at[p], ctxr.at[p], o + p, o + p, A) for p in range(2)]

        for c in range(NCH):
            ld_xo[c].wait()
            xo[rows(c), :] = xf[1, rows(c), :].astype(bf16)
            if c == 0:
                pl.semaphore_wait(bar, 2)
            snd_xb[c].start()
            ld_xs[c].wait()
            xs[rows(c), :] = xf[0, rows(c), :].astype(bf16)
            snd_xa[c].start()

        lane = lax.broadcasted_iota(jnp.int32, (1, 128), 1)
        lo = lane < 64
        even = (lane & 1) == 0

        def tables(role, r0, n):
            t = tab[role, pl.ds(r0, n), :]
            tr = pltpu.roll(t, 64, 1)
            return jnp.where(lo, t, tr), jnp.where(lo, tr, t)

        def rope(t, cs, sn):
            sw = jnp.where(even, pltpu.roll(t, 127, 1), pltpu.roll(t, 1, 1))
            return t * cs + sw * sn

        def proj_kv(xsrc, r0, n, role, kvrow):
            cs, sn = tables(role, r0, n)
            y = jnp.dot(xsrc[pl.ds(r0, n), :], wkv_b[...], preferred_element_type=f32)
            for p in range(2):
                kv[p, 0, pl.ds(kvrow, n), :] = rope(y[:, 128 * p:128 * p + 128], cs, sn).astype(bf16)
                kv[p, 1, pl.ds(kvrow, n), :] = y[:, 256 + 128 * p:256 + 128 * p + 128].astype(bf16)

        SCALE = 0.125 * 1.4426950408889634

        def proj_q(xsrc, role, blk):
            cs, sn = tables(role, 0, SQ)
            y = jnp.dot(xsrc[...], wq_b[...], preferred_element_type=f32)
            for p in range(2):
                q = rope(y[:, 128 * p:128 * p + 128], cs, sn) * SCALE
                qm[blk, p, pl.ds(0, SQ), :] = jnp.where(lo, q, 0.0).astype(bf16)
                qm[blk, p, pl.ds(SQ, SQ), :] = jnp.where(lo, 0.0, q).astype(bf16)

        def att(blk, p, r0, n, state):
            s = lax.dot_general(qm[blk, p], kv[p, 0, pl.ds(r0, n), :], NT, preferred_element_type=f32)
            mx = jnp.max(s, axis=1, keepdims=True)
            if state is None:
                m_new = mx
                e = jnp.exp2(s - m_new)
                l = jnp.sum(e, axis=1, keepdims=True)
                acc = jnp.dot(e.astype(bf16), kv[p, 1, pl.ds(r0, n), :], preferred_element_type=f32)
            else:
                m, l, acc = state
                m_new = jnp.maximum(m, mx)
                alpha = jnp.exp2(m - m_new)
                e = jnp.exp2(s - m_new)
                l = alpha * l + jnp.sum(e, axis=1, keepdims=True)
                acc = alpha * acc + jnp.dot(e.astype(bf16), kv[p, 1, pl.ds(r0, n), :], preferred_element_type=f32)
            return m_new, l, acc

        def fin(state):
            m, l, acc = state
            o_ = acc / l
            return jnp.where(lo, o_[:SQ], o_[SQ:]).astype(bf16)

        ld_wk.wait()
        wkv_b[:, 0:HD] = wf[1].astype(bf16)
        ld_wv.wait()
        wkv_b[:, HD:2 * HD] = wf[2].astype(bf16)
        ld_tab.wait()
        proj_kv(xo, 0, SQ, 0, 0)

        def forward(c):
            snd_xa[c].wait_recv()
            proj_kv(xa, c * CR, CR, 1, SQ + c * CR)
            fwd[c][0].start()
            fwd[c][1].start()

        forward(0)
        ld_wq.wait()
        wq_b[...] = wf[0].astype(bf16)
        proj_q(xo, 0, 0)
        stO = [att(0, p, 0, SQ, None) for p in range(2)]
        for c in range(1, NCH):
            forward(c)
        proj_q(xa, 1, 1)
        for c in range(NCH):
            snd_xb[c].wait_recv()
        proj_kv(xb, 0, SQ, 2, 2 * SQ)
        stA = [att(1, p, 0, 3 * SQ, None) for p in range(2)]
        stO = [att(0, p, SQ, 2 * SQ, stO[p]) for p in range(2)]
        ld_wo.wait()
        wo_b[...] = wof[...].astype(bf16)

        ctxO = []
        for p in range(2):
            for c in range(NCH):
                fwd[c][p].wait_recv()
            sA = att(1, p, 3 * SQ, SQ, stA[p])
            ctxs[p] = fin(sA)
            ret[p].start()
            sO = att(0, p, 3 * SQ, SQ, stO[p])
            ctxO.append(fin(sO))
        out_ref[b] = (jnp.dot(ctxO[0], wo_b[0:128, :], preferred_element_type=f32)
                      + jnp.dot(ctxO[1], wo_b[128:256, :], preferred_element_type=f32)).astype(out_ref.dtype)
        ret[0].wait_recv()
        y0 = jnp.dot(ctxr[0], wo_b[0:128, :], preferred_element_type=f32)
        ret[1].wait_recv()
        y1 = jnp.dot(ctxr[1], wo_b[128:256, :], preferred_element_type=f32)
        out_ref[1 - b] = (y0 + y1).astype(out_ref.dtype)

        for c in range(NCH):
            snd_xa[c].wait_send()
            snd_xb[c].wait_send()
            for p in range(2):
                fwd[c][p].wait_send()
        for p in range(2):
            ret[p].wait_send()

    nsem = 4 * NCH + 2
    return pl.pallas_call(
        body,
        out_shape=jax.ShapeDtypeStruct((2, SQ, DM), f32),
        in_specs=[pl.BlockSpec(memory_space=pl.ANY)] * 6,
        out_specs=pl.BlockSpec(memory_space=pltpu.VMEM),
        scratch_shapes=[
            pltpu.VMEM((2, SQ, DM), f32),
            pltpu.VMEM((SQ, DM), bf16),
            pltpu.VMEM((SQ, DM), bf16),
            pltpu.VMEM((SQ, DM), bf16),
            pltpu.VMEM((SQ, DM), bf16),
            pltpu.VMEM((3, DM, HD), f32),
            pltpu.VMEM((HD, DM), f32),
            pltpu.VMEM((DM, HD), bf16),
            pltpu.VMEM((DM, 2 * HD), bf16),
            pltpu.VMEM((HD, DM), bf16),
            pltpu.VMEM((3, SQ, 128), f32),
            pltpu.VMEM((2, 2, 4 * SQ, 128), bf16),
            pltpu.VMEM((2, 2, 2 * SQ, 128), bf16),
            pltpu.VMEM((2, SQ, 128), bf16),
            pltpu.VMEM((2, SQ, 128), bf16),
            pltpu.SemaphoreType.DMA((2 * NCH + 5,)),
            pltpu.SemaphoreType.DMA((nsem,)),
            pltpu.SemaphoreType.DMA((nsem,)),
        ],
        compiler_params=pltpu.CompilerParams(collective_id=0, vmem_limit_bytes=64 * 1024 * 1024),
    )(x, Wq, Wk, Wv, Wo, jnp.asarray(_TAB))
```

```python
import contextlib
import functools
import numpy as np
import jax
import jax.numpy as jnp
from jax import lax
from jax.experimental import pallas as pl
from jax.experimental.pallas import tpu as pltpu

SQ = 128
DM = 512
HD = 256
DH = 64

SCOPES = False
def sc(n):
    on = SCOPES if SCOPES in (True, False) else n.startswith(("wait", "xsend", "drain"))
    return jax.named_scope(n) if on else contextlib.nullcontext()


def _rope_tables():
    inv = 1.0 / (10000.0 ** (np.arange(0, DH, 2) / DH))
    pos = np.arange(4 * SQ)[:, None] * inv[None, :]
    cos = np.repeat(np.cos(pos), 2, axis=-1).astype(np.float32)
    sin = np.repeat(np.sin(pos), 2, axis=-1).astype(np.float32)
    sgn = np.where(np.arange(DH) % 2 == 0, -1.0, 1.0).astype(np.float32)
    sin = sin * sgn[None, :]
    cos = np.tile(cos, (1, 2)).reshape(4, SQ, 128)
    sin = np.tile(sin, (1, 2)).reshape(4, SQ, 128)
    t = np.stack([cos, sin], axis=1)
    out = np.stack([np.stack([t[i ^ 1], t[i], t[3 - i]]) for i in range(4)])
    return np.ascontiguousarray(out)


_TAB = _rope_tables()
RA, RO, RB = 0, 1, 2
SO, SA, SB, SD = 0, 1, 2, 3

CFG = dict(nld=4, msplit=4, out_dtype=jnp.bfloat16, nosem=True, wait_xb_early=False, pre=("o0", "wo"), safety=True, oD0_early=False)


def make_kernel(**kw):
    cfg = dict(CFG); cfg.update(kw)
    NLD = cfg["nld"]
    LR = SQ // NLD
    NF = 2
    FR = SQ // NF
    LPF = NLD // NF
    f32, bf16, i32 = jnp.float32, jnp.bfloat16, jnp.int32
    MESH = pl.DeviceIdType.MESH
    NT = (((1,), (1,)), ((), ()))
    SCALE = 0.125 * 1.4426950408889634

    def b16(v):
        return pltpu.bitcast(v, bf16)

    def c32(v):
        return pltpu.bitcast(v, i32)

    def body(x_hbm, wq_hbm, wk_hbm, wv_hbm, wo_hbm, tab_hbm, out_ref,
             xf, xs, xo, xa, xb, wf, wof, wq_b, wkv_b, wo_b, tab, kv, qm, acc_r, lp_r, ctxs, ctxr, y0_r,
             pbuf, rbuf, ctxo, ctxs2, ctxr2, lsem0, ssem, rsem):
        lsem = lsem0
        wsem = lsem0.at[pl.ds(2 * NLD, 7)]
        me = lax.axis_index("i")
        A = me ^ 1
        B = 3 - me
        b = ((me + 1) >> 1) & 1

        bar = pltpu.get_barrier_semaphore()
        pl.semaphore_signal(bar, inc=1, device_id=(A,), device_id_type=MESH)
        pl.semaphore_signal(bar, inc=1, device_id=(B,), device_id_type=MESH)

        def lrows(c):
            return pl.ds(c * LR, LR)
        ld_xo = [pltpu.make_async_copy(x_hbm.at[b, lrows(c)], xf.at[1, lrows(c)], lsem.at[c]) for c in range(NLD)]
        ld_xs = [pltpu.make_async_copy(x_hbm.at[1 - b, lrows(c)], xf.at[0, lrows(c)], lsem.at[NLD + c]) for c in range(NLD)]
        ld_wk = pltpu.make_async_copy(wk_hbm, wf.at[1], wsem.at[0])
        ld_wv = pltpu.make_async_copy(wv_hbm, wf.at[2], wsem.at[1])
        ld_wq = pltpu.make_async_copy(wq_hbm, wf.at[0], wsem.at[2])
        ld_wo = pltpu.make_async_copy(wo_hbm, wof, wsem.at[3])
        ld_tab = [pltpu.make_async_copy(tab_hbm.at[me, r], tab.at[r], wsem.at[4 + r]) for r in range(3)]
        for c in range(NLD):
            ld_xo[c].start()
            ld_xs[c].start()
        ld_wk.start(); ld_wv.start(); ld_tab[RA].start(); ld_tab[RO].start(); ld_wq.start(); ld_tab[RB].start(); ld_wo.start()

        def rcopy(src, dst, si, ri, dev):
            return pltpu.make_async_remote_copy(src, dst, ssem.at[si], rsem.at[ri], device_id=(dev,), device_id_type=MESH)
        snd_xa = [rcopy(xs.at[c], xa.at[c], 0, c // LPF, A) for c in range(NLD)]
        snd_xb = [rcopy(xo.at[c], xb.at[c], 1, NF, B) for c in range(NLD)]
        F0 = NF + 1
        fwd = [[rcopy(kv.at[SA, 0], kv.at[SD, 0], 2, F0, B)],
               [rcopy(kv.at[SA, 1, 0], kv.at[SD, 1, 0], 2, F0 + 1, B),
                rcopy(kv.at[SA, 1, 1, 0], kv.at[SD, 1, 1, 0], 2, F0 + 2, B),
                rcopy(kv.at[SA, 1, 1, 1], kv.at[SD, 1, 1, 1], 2, F0 + 3, B)]]
        R0 = F0 + 4
        ret = [rcopy(ctxs.at[p], ctxr.at[p], 3, R0 + p, A) for p in range(2)]
        fix = rcopy(ctxs2, ctxr2, 4, R0 + 2, A)

        def cast_x(half, dst, c):
            v = xf[half, lrows(c), :]
            for kt in range(4):
                dst[c, kt] = c32(v[:, 128 * kt:128 * kt + 128].astype(bf16))

        for c in range(NLD):
          with sc(f"xsend{c}"):
            ld_xo[c].wait()
            cast_x(1, xo, c)
            if c == 0:
                pl.semaphore_wait(bar, 2)
            snd_xb[c].start()
            ld_xs[c].wait()
            cast_x(0, xs, c)
            snd_xa[c].start()

        lane = lax.broadcasted_iota(i32, (1, 128), 1)
        lo = lane < 64

        def swap_idx(n):
            return lax.broadcasted_iota(i32, (n, 128), 1) ^ 1

        def rope(t, role, r0, n):
            cs = tab[role, 0, pl.ds(r0, n), :]
            sn = tab[role, 1, pl.ds(r0, n), :]
            return t * cs + jnp.take_along_axis(t, swap_idx(n), axis=1) * sn

        def xcat(buf, chunks):
            return jnp.concatenate(
                [jnp.concatenate([b16(buf[c, kt]) for c in chunks], axis=0) for kt in range(4)], axis=1)

        def proj_kv(buf, fc_list, role, slot):
            chunks = [c for fc in fc_list for c in range(fc * LPF, (fc + 1) * LPF)]
            x = xcat(buf, chunks)
            w = jnp.concatenate([b16(wkv_b[nt]) for nt in range(4)], axis=1)
            y = jnp.dot(x, w, preferred_element_type=f32)
            for i, fc in enumerate(fc_list):
                for p in range(2):
                    k = rope(y[FR * i:FR * (i + 1), 128 * p:128 * p + 128], role, FR * fc, FR)
                    kv[slot, fc, p, 0] = c32(k.astype(bf16))
                    kv[slot, fc, p, 1] = c32(y[FR * i:FR * (i + 1), 256 + 128 * p:256 + 128 * p + 128].astype(bf16))

        def proj_q(buf, role, blk):
            x = xcat(buf, range(NLD))
            w = jnp.concatenate([b16(wq_b[nt]) for nt in range(2)], axis=1)
            y = jnp.dot(x, w, preferred_element_type=f32)
            for p in range(2):
                q = c32((rope(y[:, 128 * p:128 * p + 128], role, 0, SQ) * SCALE).astype(bf16))
                qm[blk, p, pl.ds(0, 64), :] = jnp.where(lo, q, 0)
                qm[blk, p, pl.ds(64, 64), :] = jnp.where(lo, 0, q)

        def kvcat(p, which, slots):
            return jnp.concatenate([b16(kv[s, c, p, which]) for s in slots for c in range(NF)], axis=0)

        def att(blk, p, slots, first):
            s = lax.dot_general(b16(qm[blk, p]), kvcat(p, 0, slots), NT, preferred_element_type=f32)
            e = jnp.exp2(s)
            lp = e[:, 0:128]
            for j in range(1, len(slots)):
                lp = lp + e[:, 128 * j:128 * j + 128]
            a = jnp.dot(e.astype(bf16), kvcat(p, 1, slots), preferred_element_type=f32)
            if first:
                acc_r[blk, p] = a
                lp_r[blk, p] = lp
            else:
                acc_r[blk, p] += a
                lp_r[blk, p] += lp

        def fin_qk(blk, p):
            k = kvcat(p, 0, [SD])
            es, ls = [], []
            for j in range(4):
                s = lax.dot_general(b16(qm[blk, p, pl.ds(32 * j, 32), :]), k, NT, preferred_element_type=f32)
                e = jnp.exp2(s)
                es.append(e.astype(bf16))
                ls.append(jnp.sum(lp_r[blk, p, pl.ds(64 * j, 64), :] + e, axis=1, keepdims=True))
            rs = []
            for h in range(2):
                lsel = jnp.where(lo, ls[h], ls[2 + h])
                r = pl.reciprocal(lsel, approx=True)
                if cfg["safety"]:
                    ok = (lsel >= 2.0 ** -80) & (lsel <= 2.0 ** 120)
                    r = jnp.where(ok, r, jnp.nan)
                rs.append(r)
            return es, rs

        def fin_pv(blk, p, es, rs, dst):
            v = kvcat(p, 1, [SD])
            accs = [acc_r[blk, p, pl.ds(64 * j, 64), :] + jnp.dot(es[j], v, preferred_element_type=f32)
                    for j in range(4)]
            for h in range(2):
                dst[p, pl.ds(32 * h, 32), :] = c32((jnp.where(lo, accs[h], accs[2 + h]) * rs[h]).astype(bf16))

        def exact(blk, p):
            slots = [SO, SA, SB, SD]
            s = lax.dot_general(b16(qm[blk, p]), kvcat(p, 0, slots), NT, preferred_element_type=f32)
            m = jnp.max(s, axis=1, keepdims=True)
            e = jnp.exp2(s - m)
            l = jnp.sum(e, axis=1, keepdims=True)
            acc = jnp.dot(e.astype(bf16), kvcat(p, 1, slots), preferred_element_type=f32)
            o = acc / l
            return jnp.where(lo, o[:SQ], o[SQ:]).astype(bf16)

        def nonfinite(ref, pairs=(0, 1)):
            bad = None
            for p in pairs:
                w = ref[p]
                nf = ((w & 0x7F80) == 0x7F80) | ((w & 0x7F800000) == 0x7F800000)
                bad = nf if bad is None else bad | nf
            return jnp.max(jnp.where(bad, 1, 0)) > 0

        def conv_w(src, dst, ntiles, nrows):
            for nt in range(ntiles):
                dst[nt] = c32(src[:, 128 * nt:128 * nt + 128].astype(bf16))

        with sc("wait_wkv"):
            ld_wk.wait()
            ld_wv.wait()
            ld_tab[RA].wait()
        with sc("conv_wkv"):
            for nt in range(2):
                wkv_b[nt] = c32(wf[1, :, 128 * nt:128 * nt + 128].astype(bf16))
                wkv_b[2 + nt] = c32(wf[2, :, 128 * nt:128 * nt + 128].astype(bf16))

        def wait_xa(fc):
            pltpu.make_async_copy(xa.at[pl.ds(fc * LPF, LPF)], xa.at[pl.ds(fc * LPF, LPF)], rsem.at[fc]).wait()

        def forward(fc):
            with sc(f"wait_xa{fc}"):
                wait_xa(fc)
            with sc(f"fwd{fc}"):
                proj_kv(xa, [fc], RA, SA)
                for c in fwd[fc]:
                    c.start()

        forward(0)
        with sc("wait_wq"):
            ld_tab[RO].wait()
            ld_wq.wait()
        with sc("kvO_qO_attOO"):
            proj_kv(xo, range(NF), RO, SO)
            for nt in range(2):
                wq_b[nt] = c32(wf[0, :, 128 * nt:128 * nt + 128].astype(bf16))
            proj_q(xo, RO, 0)
            for p in range(2):
                att(0, p, [SO], True)
        forward(1)

        def wait_xb():
            pltpu.make_async_copy(xb, xb, rsem.at[NF]).wait()
            ld_tab[RB].wait()

        if cfg["wait_xb_early"]:
            with sc("wait_xb"):
                wait_xb()
        with sc("qA"):
            proj_q(xa, RA, 1)
        if not cfg["wait_xb_early"]:
            with sc("wait_xb"):
                wait_xb()
        with sc("kvB_attA"):
            proj_kv(xb, range(NF), RB, SB)
            for p in range(2):
                att(1, p, [SO, SA, SB], True)

        def conv_wo():
            with sc("wo"):
                ld_wo.wait()
                for nt in range(4):
                    wo_b[nt] = c32(wof[:, 128 * nt:128 * nt + 128].astype(bf16))

        def owork(name):
            if name == "wo":
                conv_wo()
            else:
                with sc("attO_AB" + name):
                    att(0, int(name[1]), [SA, SB], False)

        for t in cfg["pre"]:
            owork(t)

        def wo_rows(p):
            return jnp.concatenate([b16(wo_b[nt, pl.ds(64 * p, 64), :]) for nt in range(4)], axis=1)

        def proj_o(c0, c1):
            return (jnp.dot(c0, wo_rows(0), preferred_element_type=f32)
                    + jnp.dot(c1, wo_rows(1), preferred_element_type=f32))

        with sc("wait_D0"):
            fwd[0][0].wait_recv()
            fwd[1][0].wait_recv()
        with sc("attA_D0"):
            e, r = fin_qk(1, 0)
            fin_pv(1, 0, e, r, ctxs)
            ret[0].start()
        if cfg["oD0_early"]:
            with sc("attO_D0"):
                e, r = fin_qk(0, 0)
                fin_pv(0, 0, e, r, ctxo)
        with sc("wait_K1"):
            fwd[1][1].wait_recv()
        with sc("qkA_D1"):
            e, r = fin_qk(1, 1)
            for j in range(4):
                pbuf[j] = c32(e[j])
            for h in range(2):
                rbuf[h] = r[h]
        with sc("wait_V1"):
            fwd[1][2].wait_recv()
        with sc("pvA_D1"):
            fin_pv(1, 1, [b16(pbuf[j]) for j in range(4)], [rbuf[h] for h in range(2)], ctxs)
            ret[1].start()
        for t in ("o0", "o1", "wo"):
            if t not in cfg["pre"]:
                owork(t)
        with sc("attO_D"):
            for p in range(2):
                if p == 0 and cfg["oD0_early"]:
                    continue
                e, r = fin_qk(0, p)
                fin_pv(0, p, e, r, ctxo)
        with sc("outO"):
            out_ref[b] = proj_o(b16(ctxo[0]), b16(ctxo[1])).astype(out_ref.dtype)
        if cfg["safety"]:
            with sc("check"):
                bad_s = nonfinite(ctxs)
                bad_o = nonfinite(ctxo)

                @pl.when(bad_s | bad_o)
                def _():
                    @pl.when(bad_s)
                    def _():
                        for p in range(2):
                            ctxs2[p] = c32(exact(1, p))
                        fix.start()
                        fix.wait_send()

                    @pl.when(bad_o)
                    def _():
                        out_ref[b] = proj_o(exact(0, 0), exact(0, 1)).astype(out_ref.dtype)
        with sc("wait_ret0"):
            ret[0].wait_recv()
        with sc("y0"):
            y0_r[...] = jnp.dot(b16(ctxr[0]), wo_rows(0), preferred_element_type=f32)
            if cfg["safety"]:
                bad_r0 = nonfinite(ctxr, (0,))
        with sc("wait_ret1"):
            ret[1].wait_recv()
        with sc("y1"):
            y1 = jnp.dot(b16(ctxr[1]), wo_rows(1), preferred_element_type=f32)
            out_ref[1 - b] = (y0_r[...] + y1).astype(out_ref.dtype)
            if cfg["safety"]:
                @pl.when(bad_r0 | nonfinite(ctxr, (1,)))
                def _():
                    fix.wait_recv()
                    out_ref[1 - b] = proj_o(b16(ctxr2[0]), b16(ctxr2[1])).astype(out_ref.dtype)

        with sc("drain"):
            pltpu.make_async_copy(xs, xs, ssem.at[0]).wait()
            pltpu.make_async_copy(xo, xo, ssem.at[1]).wait()
            pltpu.make_async_copy(kv.at[SA], kv.at[SA], ssem.at[2]).wait()
            pltpu.make_async_copy(ctxs, ctxs, ssem.at[3]).wait()

    def kernel_fn(x, Wq, Wk, Wv, Wo):
        XB = (NLD, 4, LR // 2, 128)
        return pl.pallas_call(
            body,
            out_shape=jax.ShapeDtypeStruct((2, SQ, DM), cfg["out_dtype"]),
            in_specs=[pl.BlockSpec(memory_space=pl.ANY)] * 6,
            out_specs=pl.BlockSpec(memory_space=pltpu.VMEM),
            scratch_shapes=[
                pltpu.VMEM((2, SQ, DM), f32),
                pltpu.VMEM(XB, i32),
                pltpu.VMEM(XB, i32),
                pltpu.VMEM(XB, i32),
                pltpu.VMEM(XB, i32),
                pltpu.VMEM((3, DM, HD), f32),
                pltpu.VMEM((HD, DM), f32),
                pltpu.VMEM((2, DM // 2, 128), i32),
                pltpu.VMEM((4, DM // 2, 128), i32),
                pltpu.VMEM((4, HD // 2, 128), i32),
                pltpu.VMEM((3, 2, SQ, 128), f32),
                pltpu.VMEM((4, NF, 2, 2, FR // 2, 128), i32),
                pltpu.VMEM((2, 2, SQ, 128), i32),
                pltpu.VMEM((2, 2, 2 * SQ, 128), f32),
                pltpu.VMEM((2, 2, 2 * SQ, 128), f32),
                pltpu.VMEM((2, SQ // 2, 128), i32),
                pltpu.VMEM((2, SQ // 2, 128), i32),
                pltpu.VMEM((SQ, DM), f32),
                pltpu.VMEM((4, 32, 128), i32),
                pltpu.VMEM((2, 64, 128), f32),
                pltpu.VMEM((2, SQ // 2, 128), i32),
                pltpu.VMEM((2, SQ // 2, 128), i32),
                pltpu.VMEM((2, SQ // 2, 128), i32),
                pltpu.SemaphoreType.DMA((2 * NLD + 7,)),
                pltpu.SemaphoreType.DMA((5,)),
                pltpu.SemaphoreType.DMA((NF + 1 + 4 + 3,)),
            ],
            compiler_params=pltpu.CompilerParams(collective_id=0, vmem_limit_bytes=64 * 1024 * 1024,
                                                 disable_semaphore_checks=cfg["nosem"]),
        )(x, Wq, Wk, Wv, Wo, jnp.asarray(_TAB))
    return kernel_fn


pallas_dist_rope_attn_qseq_b2_sq128_d512_hq4_dh64_kernel = make_kernel()
```

```python
import numpy as np
import jax
import jax.numpy as jnp
from jax import lax
from jax.experimental import pallas as pl
from jax.experimental.pallas import tpu as pltpu

SQ = 128
DM = 512
HD = 256
DH = 64
NLD = 4
LR = SQ // NLD
RA, RO, RB = 0, 1, 2
SO, SA, SB, SD = 0, 1, 2, 3
SCALE = 0.125 * 1.4426950408889634


def _rope_tables():
    inv = 1.0 / (10000.0 ** (np.arange(0, DH, 2) / DH))
    pos = np.arange(4 * SQ)[:, None] * inv[None, :]
    cos = np.repeat(np.cos(pos), 2, axis=-1).astype(np.float32)
    sin = np.repeat(np.sin(pos), 2, axis=-1).astype(np.float32)
    sin = sin * np.where(np.arange(DH) % 2 == 0, -1.0, 1.0).astype(np.float32)[None, :]
    cos = np.tile(cos, (1, 2)).reshape(4, SQ, 128)
    sin = np.tile(sin, (1, 2)).reshape(4, SQ, 128)
    t = np.stack([cos, sin], axis=1)
    return np.ascontiguousarray(np.stack([np.stack([t[i ^ 1], t[i], t[3 - i]]) for i in range(4)]))


_TAB = _rope_tables()
f32, bf16, i32 = jnp.float32, jnp.bfloat16, jnp.int32
NT = (((1,), (1,)), ((), ()))


def b16(v):
    return pltpu.bitcast(v, bf16)


def c32(v):
    return pltpu.bitcast(v, i32)


def _body(x_hbm, wq_hbm, wk_hbm, wv_hbm, wo_hbm, tab_hbm, out_ref,
          xf, xs, xo, xa, xb, wf, wof, wq_b, wkv_b, wo_b, tab, kv, kvd, qm, acc_r, lp_r, ctxs, ctxr, y0_r,
          pbuf, rbuf, ctxo, ctxs2, ctxr2, xr, kvr, lsem, ssem, rsem, ready):
    me = lax.axis_index("i")
    A = me ^ 1
    B = 3 - me
    b = ((me + 1) >> 1) & 1

    def dev(d):
        return dict(device_id=d, device_id_type=pl.DeviceIdType.LOGICAL)

    bar = pltpu.get_barrier_semaphore()

    @pl.when(me != 2)
    def _():
        pl.semaphore_signal(bar, inc=1, **dev(A))
        pl.semaphore_signal(bar, inc=1, **dev(B))

    def lrows(c):
        return pl.ds(c * LR, LR)
    ld_xo = [pltpu.make_async_copy(x_hbm.at[b, lrows(c)], xf.at[1, lrows(c)], lsem.at[c]) for c in range(NLD)]
    ld_xs = [pltpu.make_async_copy(x_hbm.at[1 - b, lrows(c)], xf.at[0, lrows(c)], lsem.at[NLD + c])
             for c in range(NLD)]
    o = 2 * NLD
    ld_wk = pltpu.make_async_copy(wk_hbm, wf.at[1], lsem.at[o])
    ld_wv = pltpu.make_async_copy(wv_hbm, wf.at[2], lsem.at[o + 1])
    ld_wq = pltpu.make_async_copy(wq_hbm, wf.at[0], lsem.at[o + 2])
    ld_wo = pltpu.make_async_copy(wo_hbm, wof, lsem.at[o + 3])
    ld_tab = [pltpu.make_async_copy(tab_hbm.at[me, r], tab.at[r], lsem.at[o + 4 + r]) for r in range(3)]
    for c in range(NLD):
        ld_xo[c].start()
        ld_xs[c].start()
    for d in (ld_wk, ld_wv, ld_tab[RA], ld_tab[RB], ld_tab[RO], ld_wq, ld_wo):
        d.start()

    def rcopy(src, dst, si, ri, to):
        return pltpu.make_async_remote_copy(src, dst, ssem.at[si], rsem.at[ri], **dev(to))
    snd_xa = [rcopy(xs.at[c], xa.at[c], 0, (0, 0, 1, 2)[c], A) for c in range(NLD)]
    snd_xb = [rcopy(xo.at[c], xb.at[c], 1, 3, B) for c in range(NLD)]
    al = slice(None)
    r0, r2, r3, r23, r02 = pl.ds(0, 32), pl.ds(32, 16), pl.ds(48, 16), pl.ds(32, 32), pl.ds(0, 48)

    def fcopy(p, which, rows, sem):
        return rcopy(kv.at[SA, p, which, rows], kvd.at[p, which, rows], 2, sem, B)
    f_a = [fcopy(0, al, r0, 4)]
    f_b = [fcopy(0, al, r2, 4), fcopy(1, 0, r0, 5), fcopy(1, 1, r0, 6)]
    f_c = [fcopy(0, al, r3, 4), fcopy(1, 0, r23, 5), fcopy(1, 1, r23, 6)]
    f_b2 = [fcopy(0, al, r2, 4), fcopy(1, 0, r0, 5), fcopy(1, 0, r2, 5), fcopy(1, 1, r0, 6), fcopy(1, 1, r2, 6)]
    rel_x = rcopy(xs.at[NLD - 1], xr, 5, 10, B)
    rel_kv = [rcopy(kvr.at[0], kvd.at[0, al, r3], 6, 4, A),
              rcopy(kvr.at[1, 0], kvd.at[1, 0, r3], 6, 5, A),
              rcopy(kvr.at[1, 1], kvd.at[1, 1, r3], 6, 6, A)]
    ret = [rcopy(ctxs.at[p], ctxr.at[p], 3, 7 + p, A) for p in range(2)]
    fix = rcopy(ctxs2, ctxr2, 4, 9, A)

    def rwait(ref, sem):
        pltpu.make_async_copy(ref, ref, rsem.at[sem]).wait()

    def swait(ref, sem):
        pltpu.make_async_copy(ref, ref, ssem.at[sem]).wait()

    def cast_x(half, dst, c):
        v = xf[half, lrows(c), :]
        for kt in range(4):
            dst[c, kt] = c32(v[:, 128 * kt:128 * kt + 128].astype(bf16))

    even = (me & 1) == 0
    pl.when(even)(lambda: pl.semaphore_wait(bar, 2))
    pl.when(jnp.logical_not(even))(lambda: pl.semaphore_wait(bar, 1))

    @pl.when(me == 2)
    def _():
        pl.semaphore_signal(ready, inc=1, **dev(A))
        pl.semaphore_signal(ready, inc=1, **dev(B))

    for c in range(NLD):
        ld_xo[c].wait()
        cast_x(1, xo, c)
        pl.when(me != 1)(snd_xb[c].start)
        if c == 1:
            @pl.when(me == 3)
            def _():
                ld_xs[NLD - 1].wait()
                cast_x(0, xs, NLD - 1)
                rel_x.start()
        if c == NLD - 1:
            @pl.when(me != 3)
            def _():
                ld_xs[c].wait()
                cast_x(0, xs, c)
        else:
            ld_xs[c].wait()
            cast_x(0, xs, c)
        pl.when(me != 3)(snd_xa[c].start)

    @pl.when(me == 1)
    def _():
        pl.semaphore_wait(ready, 1)
        for d in snd_xb:
            d.start()

    @pl.when(me == 3)
    def _():
        pl.semaphore_wait(ready, 1)
        for d in snd_xa:
            d.start()

    lo = lax.broadcasted_iota(i32, (1, 128), 1) < 64

    def rope(t, role, row0, n):
        cs = tab[role, 0, pl.ds(row0, n), :]
        sn = tab[role, 1, pl.ds(row0, n), :]
        swap = lax.broadcasted_iota(i32, (n, 128), 1) ^ 1
        return t * cs + jnp.take_along_axis(t, swap, axis=1) * sn

    def xcat(buf, chunks):
        return jnp.concatenate(
            [jnp.concatenate([b16(buf[c, kt]) for c in chunks], axis=0) for kt in range(4)], axis=1)

    def proj_kv(x, role, row0, n, store):
        w = jnp.concatenate([b16(wkv_b[nt]) for nt in range(4)], axis=1)
        y = jnp.dot(x, w, preferred_element_type=f32)
        for p in range(2):
            store(p, 0, c32(rope(y[:, 128 * p:128 * p + 128], role, row0, n).astype(bf16)))
            store(p, 1, c32(y[:, 256 + 128 * p:256 + 128 * p + 128].astype(bf16)))

    def proj_slot(buf, chunks, role, slot):
        row0, n = chunks[0] * LR, len(chunks) * LR

        def store(p, which, v):
            kv[slot, p, which, pl.ds(row0 // 2, n // 2), :] = v
        proj_kv(xcat(buf, chunks), role, row0, n, store)

    def proj_q(buf, role, blk):
        x = xcat(buf, range(NLD))
        w = jnp.concatenate([b16(wq_b[nt]) for nt in range(2)], axis=1)
        y = jnp.dot(x, w, preferred_element_type=f32)
        for p in range(2):
            q = c32((rope(y[:, 128 * p:128 * p + 128], role, 0, SQ) * SCALE).astype(bf16))
            qm[blk, p, pl.ds(0, 64), :] = jnp.where(lo, q, 0)
            qm[blk, p, pl.ds(64, 64), :] = jnp.where(lo, 0, q)

    def kvcat(p, which, slots):
        return jnp.concatenate([b16(kvd[p, which] if s == SD else kv[s, p, which]) for s in slots], axis=0)

    def att(blk, p, slots, first):
        s = lax.dot_general(b16(qm[blk, p]), kvcat(p, 0, slots), NT, preferred_element_type=f32)
        e = jnp.exp2(s)
        lp = e[:, 0:128]
        for j in range(1, len(slots)):
            lp = lp + e[:, 128 * j:128 * j + 128]
        a = jnp.dot(e.astype(bf16), kvcat(p, 1, slots), preferred_element_type=f32)
        if first:
            acc_r[blk, p] = a
            lp_r[blk, p] = lp
        else:
            acc_r[blk, p] += a
            lp_r[blk, p] += lp

    def fin_qk(blk, p):
        k = kvcat(p, 0, [SD])
        es, ls = [], []
        for j in range(4):
            s = lax.dot_general(b16(qm[blk, p, pl.ds(32 * j, 32), :]), k, NT, preferred_element_type=f32)
            e = jnp.exp2(s)
            es.append(e.astype(bf16))
            ls.append(jnp.sum(lp_r[blk, p, pl.ds(64 * j, 64), :] + e, axis=1, keepdims=True))
        rs = []
        for h in range(2):
            lsel = jnp.where(lo, ls[h], ls[2 + h])
            ok = (lsel >= 2.0 ** -80) & (lsel <= 2.0 ** 120)
            rs.append(jnp.where(ok, pl.reciprocal(lsel, approx=True), jnp.nan))
        return es, rs

    def fin_pv(blk, p, es, rs, dst):
        v = kvcat(p, 1, [SD])
        accs = [acc_r[blk, p, pl.ds(64 * j, 64), :] + jnp.dot(es[j], v, preferred_element_type=f32)
                for j in range(4)]
        for h in range(2):
            dst[p, pl.ds(32 * h, 32), :] = c32((jnp.where(lo, accs[h], accs[2 + h]) * rs[h]).astype(bf16))

    def exact(blk, p):
        slots = [SO, SA, SB, SD]
        s = lax.dot_general(b16(qm[blk, p]), kvcat(p, 0, slots), NT, preferred_element_type=f32)
        e = jnp.exp2(s - jnp.max(s, axis=1, keepdims=True))
        l = jnp.sum(e, axis=1, keepdims=True)
        o_ = jnp.dot(e.astype(bf16), kvcat(p, 1, slots), preferred_element_type=f32) / l
        return jnp.where(lo, o_[:SQ], o_[SQ:]).astype(bf16)

    def nonfinite(ref, pairs=(0, 1)):
        bad = None
        for p in pairs:
            w = ref[p]
            nf = ((w & 0x7F80) == 0x7F80) | ((w & 0x7F800000) == 0x7F800000)
            bad = nf if bad is None else bad | nf
        return jnp.max(jnp.where(bad, 1, 0))

    for d in (ld_wk, ld_wv, ld_tab[RA], ld_tab[RB]):
        d.wait()
    for nt in range(2):
        wkv_b[nt] = c32(wf[1, :, 128 * nt:128 * nt + 128].astype(bf16))
        wkv_b[2 + nt] = c32(wf[2, :, 128 * nt:128 * nt + 128].astype(bf16))

    rwait(xa.at[pl.ds(0, 2)], 0)
    proj_slot(xa, [0, 1], RA, SA)
    for d in f_a:
        d.start()
    ld_tab[RO].wait()
    proj_slot(xo, range(NLD), RO, SO)

    @pl.when(me == 0)
    def _():
        rwait(xr, 10)

        def store(p, which, v):
            kvr[p, which] = v
        proj_kv(jnp.concatenate([b16(xr[kt]) for kt in range(4)], axis=1), RB, SQ - LR, LR, store)
        for d in rel_kv:
            d.start()

    rwait(xa.at[2], 1)
    proj_slot(xa, [2], RA, SA)

    @pl.when(me == 2)
    def _():
        for d in f_b2:
            d.start()

    @pl.when(me != 2)
    def _():
        for d in f_b:
            d.start()

    ld_wq.wait()
    for nt in range(2):
        wq_b[nt] = c32(wf[0, :, 128 * nt:128 * nt + 128].astype(bf16))

    def q_oo():
        proj_q(xo, RO, 0)
        for p in range(2):
            att(0, p, [SO], True)

    def o_ab():
        for p in range(2):
            att(0, p, [SA, SB], False)

    def o_fin(p):
        es, rs = fin_qk(0, p)
        fin_pv(0, p, es, rs, ctxo)

    pl.when(me != 1)(q_oo)
    rwait(xa.at[3], 2)
    proj_slot(xa, [3], RA, SA)

    @pl.when(me != 2)
    def _():
        for d in f_c:
            d.start()

    def mid(with_o):
        rwait(xb, 3)
        proj_q(xa, RA, 1)
        proj_slot(xb, range(NLD), RB, SB)
        for p in range(2):
            att(1, p, [SO, SA, SB], True)
        if with_o:
            o_ab()

    pl.when(me != 1)(lambda: mid(True))
    pl.when(me == 1)(lambda: mid(False))
    ld_wo.wait()
    for nt in range(4):
        wo_b[nt] = c32(wof[:, 128 * nt:128 * nt + 128].astype(bf16))

    def wo_rows(p):
        return jnp.concatenate([b16(wo_b[nt, pl.ds(64 * p, 64), :]) for nt in range(4)], axis=1)

    def proj_o(c0, c1):
        return (jnp.dot(c0, wo_rows(0), preferred_element_type=f32)
                + jnp.dot(c1, wo_rows(1), preferred_element_type=f32))

    rwait(kvd.at[0], 4)
    es, rs = fin_qk(1, 0)
    fin_pv(1, 0, es, rs, ctxs)
    ret[0].start()
    pl.when(me != 1)(lambda: o_fin(0))
    rwait(kvd.at[1, 0], 5)
    es, rs = fin_qk(1, 1)
    for j in range(4):
        pbuf[j] = c32(es[j])
    for h in range(2):
        rbuf[h] = rs[h]
    rwait(kvd.at[1, 1], 6)
    fin_pv(1, 1, [b16(pbuf[j]) for j in range(4)], [rbuf[h] for h in range(2)], ctxs)
    ret[1].start()

    swait(xs, 0)
    swait(xo, 1)
    pl.when(me == 2)(lambda: swait(kv.at[SA, al, al, r02], 2))
    pl.when(me != 2)(lambda: swait(kv.at[SA], 2))
    pl.when(me == 3)(lambda: swait(xr, 5))
    pl.when(me == 0)(lambda: swait(kvr, 6))

    def tail(is_late):
        if is_late:
            q_oo()
            o_ab()
            o_fin(0)
        else:
            ret[0].wait_recv()
        o_fin(1)
        out_ref[b] = proj_o(b16(ctxo[0]), b16(ctxo[1])).astype(out_ref.dtype)
        if is_late:
            ret[0].wait_recv()
        y0_r[...] = jnp.dot(b16(ctxr[0]), wo_rows(0), preferred_element_type=f32)
        return nonfinite(ctxs), nonfinite(ctxo), nonfinite(ctxr, (0,))

    bad_s, bad_o, bad_r0 = lax.cond(me == 1, lambda: tail(True), lambda: tail(False))

    @pl.when(bad_s + bad_o > 0)
    def _():
        @pl.when(bad_s > 0)
        def _():
            for p in range(2):
                ctxs2[p] = c32(exact(1, p))
            fix.start()
            fix.wait_send()

        @pl.when(bad_o > 0)
        def _():
            out_ref[b] = proj_o(exact(0, 0), exact(0, 1)).astype(out_ref.dtype)

    ret[1].wait_recv()
    y1 = jnp.dot(b16(ctxr[1]), wo_rows(1), preferred_element_type=f32)
    out_ref[1 - b] = (y0_r[...] + y1).astype(out_ref.dtype)

    @pl.when(bad_r0 + nonfinite(ctxr, (1,)) > 0)
    def _():
        fix.wait_recv()
        out_ref[1 - b] = proj_o(b16(ctxr2[0]), b16(ctxr2[1])).astype(out_ref.dtype)

    swait(ctxs, 3)


def pallas_dist_rope_attn_qseq_b2_sq128_d512_hq4_dh64_kernel(x, Wq, Wk, Wv, Wo):
    XB = (NLD, 4, LR // 2, 128)
    CB = (2, SQ // 2, 128)
    return pl.pallas_call(
        _body,
        out_shape=jax.ShapeDtypeStruct((2, SQ, DM), bf16),
        in_specs=[pl.BlockSpec(memory_space=pl.ANY)] * 6,
        out_specs=pl.BlockSpec(memory_space=pltpu.VMEM),
        scratch_shapes=[
            pltpu.VMEM((2, SQ, DM), f32),
            pltpu.VMEM(XB, i32),
            pltpu.VMEM(XB, i32),
            pltpu.VMEM(XB, i32),
            pltpu.VMEM(XB, i32),
            pltpu.VMEM((3, DM, HD), f32),
            pltpu.VMEM((HD, DM), f32),
            pltpu.VMEM((2, DM // 2, 128), i32),
            pltpu.VMEM((4, DM // 2, 128), i32),
            pltpu.VMEM((4, HD // 2, 128), i32),
            pltpu.VMEM((3, 2, SQ, 128), f32),
            pltpu.VMEM((3, 2, 2, SQ // 2, 128), i32),
            pltpu.VMEM((2, 2, SQ // 2, 128), i32),
            pltpu.VMEM((2, 2, SQ, 128), i32),
            pltpu.VMEM((2, 2, 2 * SQ, 128), f32),
            pltpu.VMEM((2, 2, 2 * SQ, 128), f32),
            pltpu.VMEM(CB, i32),
            pltpu.VMEM(CB, i32),
            pltpu.VMEM((SQ, DM), f32),
            pltpu.VMEM((4, 32, 128), i32),
            pltpu.VMEM((2, 64, 128), f32),
            pltpu.VMEM(CB, i32),
            pltpu.VMEM(CB, i32),
            pltpu.VMEM(CB, i32),
            pltpu.VMEM((4, LR // 2, 128), i32),
            pltpu.VMEM((2, 2, LR // 2, 128), i32),
            pltpu.SemaphoreType.DMA((2 * NLD + 7,)),
            pltpu.SemaphoreType.DMA((7,)),
            pltpu.SemaphoreType.DMA((11,)),
            pltpu.SemaphoreType.REGULAR,
        ],
        compiler_params=pltpu.CompilerParams(
            collective_id=0, vmem_limit_bytes=64 * 1024 * 1024, disable_semaphore_checks=True),
    )(x, Wq, Wk, Wv, Wo, jnp.asarray(_TAB))
```

```python
import numpy as np
import jax
import jax.numpy as jnp
from jax import lax
from jax.experimental import pallas as pl
from jax.experimental.pallas import tpu as pltpu

SQ = 128
DM = 512
HD = 256
DH = 64
NLD = 4
LR = SQ // NLD
RA, RO, RB = 0, 1, 2
SO, SA, SB, SD = 0, 1, 2, 3
SCALE = 0.125 * 1.4426950408889634


def _rope_tables():
    inv = 1.0 / (10000.0 ** (np.arange(0, DH, 2) / DH))
    pos = np.arange(4 * SQ)[:, None] * inv[None, :]
    cos = np.repeat(np.cos(pos), 2, axis=-1).astype(np.float32)
    sin = np.repeat(np.sin(pos), 2, axis=-1).astype(np.float32)
    sin = sin * np.where(np.arange(DH) % 2 == 0, -1.0, 1.0).astype(np.float32)[None, :]
    cos = np.tile(cos, (1, 2)).reshape(4, SQ, 128)
    sin = np.tile(sin, (1, 2)).reshape(4, SQ, 128)
    t = np.stack([cos, sin], axis=1)
    return np.ascontiguousarray(np.stack([np.stack([t[i ^ 1], t[i], t[3 - i]]) for i in range(4)]))


_TAB = _rope_tables()
f32, bf16, i32 = jnp.float32, jnp.bfloat16, jnp.int32
NT = (((1,), (1,)), ((), ()))


def b16(v):
    return pltpu.bitcast(v, bf16)


def c32(v):
    return pltpu.bitcast(v, i32)


def _body(x_hbm, wq_hbm, wk_hbm, wv_hbm, wo_hbm, tab_hbm, out_ref,
          xf, xs, xo, xa, xb, wf, wof, wq_b, wkv_b, wo_b, tab, kv, kvd, qm, acc_r, lp_r, ctxs, ctxr, y0_r,
          pbuf, rbuf, ctxo, ctxs2, ctxr2, xr, kvr, lsem, ssem, rsem, ready):
    me = lax.axis_index("i")
    A = me ^ 1
    B = 3 - me
    b = ((me + 1) >> 1) & 1

    def dev(d):
        return dict(device_id=d, device_id_type=pl.DeviceIdType.LOGICAL)

    bar = pltpu.get_barrier_semaphore()

    @pl.when(me != 2)
    def _():
        pl.semaphore_signal(bar, inc=1, **dev(A))
        pl.semaphore_signal(bar, inc=1, **dev(B))

    def lrows(c):
        return pl.ds(c * LR, LR)
    ld_xo = [pltpu.make_async_copy(x_hbm.at[b, lrows(c)], xf.at[1, lrows(c)], lsem.at[c]) for c in range(NLD)]
    ld_xs = [pltpu.make_async_copy(x_hbm.at[1 - b, lrows(c)], xf.at[0, lrows(c)], lsem.at[NLD + c])
             for c in range(NLD)]
    o = 2 * NLD
    ld_wk = pltpu.make_async_copy(wk_hbm, wf.at[1], lsem.at[o])
    ld_wv = pltpu.make_async_copy(wv_hbm, wf.at[2], lsem.at[o + 1])
    ld_wq = pltpu.make_async_copy(wq_hbm, wf.at[0], lsem.at[o + 2])
    ld_wo = pltpu.make_async_copy(wo_hbm, wof, lsem.at[o + 3])
    ld_tab = [pltpu.make_async_copy(tab_hbm.at[me, r], tab.at[r], lsem.at[o + 4 + r]) for r in range(3)]
    for c in range(NLD):
        ld_xo[c].start()
        ld_xs[c].start()
    for d in (ld_wk, ld_wv, ld_tab[RA], ld_tab[RO], ld_tab[RB], ld_wq, ld_wo):
        d.start()

    def rcopy(src, dst, si, ri, to):
        return pltpu.make_async_remote_copy(src, dst, ssem.at[si], rsem.at[ri], **dev(to))
    snd_xa = [rcopy(xs.at[c], xa.at[c], 0, (0, 11, 1, 2)[c], A) for c in range(NLD)]
    snd_xb = [rcopy(xo.at[c], xb.at[c], 1, 3, B) for c in range(NLD)]
    al = slice(None)
    r0, r2, r3, r23, r02 = pl.ds(0, 32), pl.ds(32, 16), pl.ds(48, 16), pl.ds(32, 32), pl.ds(0, 48)

    def fcopy(p, which, rows, sem):
        return rcopy(kv.at[SA, p, which, rows], kvd.at[p, which, rows], 2, sem, B)
    f_a = [fcopy(0, al, r0, 4)]
    f_b = [fcopy(0, al, r2, 4), fcopy(1, 0, r0, 5), fcopy(1, 1, r0, 6)]
    f_c = [fcopy(0, al, r3, 4), fcopy(1, 0, r23, 5), fcopy(1, 1, r23, 6)]
    f_a2 = [[fcopy(0, al, pl.ds(0, 16), 4)], [fcopy(0, al, pl.ds(16, 16), 4), fcopy(1, 0, r0, 5)]]
    f_b2 = [fcopy(0, al, r2, 4), fcopy(1, 0, r2, 5), fcopy(1, 1, r0, 6), fcopy(1, 1, r2, 6)]
    rel_x = rcopy(xs.at[NLD - 1], xr, 5, 10, B)
    rel_kv = [rcopy(kvr.at[0], kvd.at[0, al, r3], 6, 4, A),
              rcopy(kvr.at[1, 0], kvd.at[1, 0, r3], 6, 5, A),
              rcopy(kvr.at[1, 1], kvd.at[1, 1, r3], 6, 6, A)]
    ret = [rcopy(ctxs.at[p], ctxr.at[p], 3, 7 + p, A) for p in range(2)]
    fix = rcopy(ctxs2, ctxr2, 4, 9, A)

    def rwait(ref, sem):
        pltpu.make_async_copy(ref, ref, rsem.at[sem]).wait()

    def swait(ref, sem):
        pltpu.make_async_copy(ref, ref, ssem.at[sem]).wait()

    def cast_x(half, dst, c):
        v = xf[half, lrows(c), :]
        for kt in range(4):
            dst[c, kt] = c32(v[:, 128 * kt:128 * kt + 128].astype(bf16))

    even = (me & 1) == 0
    pl.when(even)(lambda: pl.semaphore_wait(bar, 2))
    pl.when(jnp.logical_not(even))(lambda: pl.semaphore_wait(bar, 1))

    @pl.when(me == 2)
    def _():
        pl.semaphore_signal(ready, inc=1, **dev(A))
        pl.semaphore_signal(ready, inc=1, **dev(B))

    for c in range(NLD):
        ld_xo[c].wait()
        cast_x(1, xo, c)
        pl.when(me != 1)(snd_xb[c].start)
        if c == 1:
            @pl.when(me == 3)
            def _():
                ld_xs[NLD - 1].wait()
                cast_x(0, xs, NLD - 1)
                rel_x.start()
        if c == NLD - 1:
            @pl.when(me != 3)
            def _():
                ld_xs[c].wait()
                cast_x(0, xs, c)
        else:
            ld_xs[c].wait()
            cast_x(0, xs, c)
        pl.when(me != 3)(snd_xa[c].start)

    @pl.when(me == 1)
    def _():
        pl.semaphore_wait(ready, 1)
        for d in snd_xb:
            d.start()

    @pl.when(me == 3)
    def _():
        pl.semaphore_wait(ready, 1)
        for d in snd_xa:
            d.start()

    lo = lax.broadcasted_iota(i32, (1, 128), 1) < 64

    def rope(t, role, row0, n):
        cs = tab[role, 0, pl.ds(row0, n), :]
        sn = tab[role, 1, pl.ds(row0, n), :]
        swap = lax.broadcasted_iota(i32, (n, 128), 1) ^ 1
        return t * cs + jnp.take_along_axis(t, swap, axis=1) * sn

    def xcat(buf, chunks):
        return jnp.concatenate(
            [jnp.concatenate([b16(buf[c, kt]) for c in chunks], axis=0) for kt in range(4)], axis=1)

    def proj_kv(x, role, row0, n, store):
        w = jnp.concatenate([b16(wkv_b[nt]) for nt in range(4)], axis=1)
        y = jnp.dot(x, w, preferred_element_type=f32)
        for p in range(2):
            store(p, 0, c32(rope(y[:, 128 * p:128 * p + 128], role, row0, n).astype(bf16)))
            store(p, 1, c32(y[:, 256 + 128 * p:256 + 128 * p + 128].astype(bf16)))

    def proj_slot(buf, chunks, role, slot):
        row0, n = chunks[0] * LR, len(chunks) * LR

        def store(p, which, v):
            kv[slot, p, which, pl.ds(row0 // 2, n // 2), :] = v
        proj_kv(xcat(buf, chunks), role, row0, n, store)

    def proj_q(buf, role, blk):
        x = xcat(buf, range(NLD))
        w = jnp.concatenate([b16(wq_b[nt]) for nt in range(2)], axis=1)
        y = jnp.dot(x, w, preferred_element_type=f32)
        for p in range(2):
            q = c32((rope(y[:, 128 * p:128 * p + 128], role, 0, SQ) * SCALE).astype(bf16))
            qm[blk, p, pl.ds(0, 64), :] = jnp.where(lo, q, 0)
            qm[blk, p, pl.ds(64, 64), :] = jnp.where(lo, 0, q)

    def kvcat(p, which, slots):
        return jnp.concatenate([b16(kvd[p, which] if s == SD else kv[s, p, which]) for s in slots], axis=0)

    def att(blk, p, slots, first):
        s = lax.dot_general(b16(qm[blk, p]), kvcat(p, 0, slots), NT, preferred_element_type=f32)
        e = jnp.exp2(s)
        lp = e[:, 0:128]
        for j in range(1, len(slots)):
            lp = lp + e[:, 128 * j:128 * j + 128]
        a = jnp.dot(e.astype(bf16), kvcat(p, 1, slots), preferred_element_type=f32)
        if first:
            acc_r[blk, p] = a
            lp_r[blk, p] = lp
        else:
            acc_r[blk, p] += a
            lp_r[blk, p] += lp

    def fin_qk(blk, p):
        k = kvcat(p, 0, [SD])
        es, ls = [], []
        for j in range(4):
            s = lax.dot_general(b16(qm[blk, p, pl.ds(32 * j, 32), :]), k, NT, preferred_element_type=f32)
            e = jnp.exp2(s)
            es.append(e.astype(bf16))
            ls.append(jnp.sum(lp_r[blk, p, pl.ds(64 * j, 64), :] + e, axis=1, keepdims=True))
        rs = []
        for h in range(2):
            lsel = jnp.where(lo, ls[h], ls[2 + h])
            ok = (lsel >= 2.0 ** -80) & (lsel <= 2.0 ** 120)
            rs.append(jnp.where(ok, pl.reciprocal(lsel, approx=True), jnp.nan))
        return es, rs

    def fin_pv(blk, p, es, rs, dst):
        v = kvcat(p, 1, [SD])
        accs = [acc_r[blk, p, pl.ds(64 * j, 64), :] + jnp.dot(es[j], v, preferred_element_type=f32)
                for j in range(4)]
        for h in range(2):
            dst[p, pl.ds(32 * h, 32), :] = c32((jnp.where(lo, accs[h], accs[2 + h]) * rs[h]).astype(bf16))

    def exact(blk, p):
        slots = [SO, SA, SB, SD]
        s = lax.dot_general(b16(qm[blk, p]), kvcat(p, 0, slots), NT, preferred_element_type=f32)
        e = jnp.exp2(s - jnp.max(s, axis=1, keepdims=True))
        l = jnp.sum(e, axis=1, keepdims=True)
        o_ = jnp.dot(e.astype(bf16), kvcat(p, 1, slots), preferred_element_type=f32) / l
        return jnp.where(lo, o_[:SQ], o_[SQ:]).astype(bf16)

    def nonfinite(ref, pairs=(0, 1)):
        bad = None
        for p in pairs:
            w = ref[p]
            nf = ((w & 0x7F80) == 0x7F80) | ((w & 0x7F800000) == 0x7F800000)
            bad = nf if bad is None else bad | nf
        return jnp.max(jnp.where(bad, 1, 0))

    for d in (ld_wk, ld_wv, ld_tab[RA]):
        d.wait()
    for nt in range(2):
        wkv_b[nt] = c32(wf[1, :, 128 * nt:128 * nt + 128].astype(bf16))
        wkv_b[2 + nt] = c32(wf[2, :, 128 * nt:128 * nt + 128].astype(bf16))

    @pl.when(me != 2)
    def _():
        rwait(xa.at[0], 0)
        rwait(xa.at[1], 11)
        proj_slot(xa, [0, 1], RA, SA)
        for d in f_a:
            d.start()

    @pl.when(me == 2)
    def _():
        for c in range(2):
            rwait(xa.at[c], (0, 11)[c])
            proj_slot(xa, [c], RA, SA)
            for d in f_a2[c]:
                d.start()

    ld_tab[RO].wait()
    proj_slot(xo, range(NLD), RO, SO)
    ld_tab[RB].wait()

    @pl.when(me == 0)
    def _():
        rwait(xr, 10)

        def store(p, which, v):
            kvr[p, which] = v
        proj_kv(jnp.concatenate([b16(xr[kt]) for kt in range(4)], axis=1), RB, SQ - LR, LR, store)
        for d in rel_kv:
            d.start()

    rwait(xa.at[2], 1)
    proj_slot(xa, [2], RA, SA)

    @pl.when(me == 2)
    def _():
        for d in f_b2:
            d.start()

    @pl.when(me != 2)
    def _():
        for d in f_b:
            d.start()

    ld_wq.wait()
    for nt in range(2):
        wq_b[nt] = c32(wf[0, :, 128 * nt:128 * nt + 128].astype(bf16))

    def q_oo():
        proj_q(xo, RO, 0)
        for p in range(2):
            att(0, p, [SO], True)

    def o_ab():
        for p in range(2):
            att(0, p, [SA, SB], False)

    def o_fin(p):
        es, rs = fin_qk(0, p)
        fin_pv(0, p, es, rs, ctxo)

    pl.when(me != 1)(q_oo)
    rwait(xa.at[3], 2)
    proj_slot(xa, [3], RA, SA)

    @pl.when(me != 2)
    def _():
        for d in f_c:
            d.start()

    def mid(with_o):
        rwait(xb, 3)
        proj_q(xa, RA, 1)
        proj_slot(xb, range(NLD), RB, SB)
        for p in range(2):
            att(1, p, [SO, SA, SB], True)
        if with_o:
            o_ab()

    pl.when(me != 1)(lambda: mid(True))
    pl.when(me == 1)(lambda: mid(False))
    ld_wo.wait()
    for nt in range(4):
        wo_b[nt] = c32(wof[:, 128 * nt:128 * nt + 128].astype(bf16))

    def wo_rows(p):
        return jnp.concatenate([b16(wo_b[nt, pl.ds(64 * p, 64), :]) for nt in range(4)], axis=1)

    def proj_o(c0, c1):
        return (jnp.dot(c0, wo_rows(0), preferred_element_type=f32)
                + jnp.dot(c1, wo_rows(1), preferred_element_type=f32))

    rwait(kvd.at[0], 4)
    es, rs = fin_qk(1, 0)
    fin_pv(1, 0, es, rs, ctxs)
    ret[0].start()
    pl.when(me != 1)(lambda: o_fin(0))
    rwait(kvd.at[1, 0], 5)
    es, rs = fin_qk(1, 1)
    for j in range(4):
        pbuf[j] = c32(es[j])
    for h in range(2):
        rbuf[h] = rs[h]
    rwait(kvd.at[1, 1], 6)
    fin_pv(1, 1, [b16(pbuf[j]) for j in range(4)], [rbuf[h] for h in range(2)], ctxs)
    ret[1].start()

    swait(xs, 0)
    swait(xo, 1)
    pl.when(me == 2)(lambda: swait(kv.at[SA, al, al, r02], 2))
    pl.when(me != 2)(lambda: swait(kv.at[SA], 2))
    pl.when(me == 3)(lambda: swait(xr, 5))
    pl.when(me == 0)(lambda: swait(kvr, 6))

    def tail(is_late):
        if is_late:
            q_oo()
            o_ab()
            o_fin(0)
        else:
            ret[0].wait_recv()
        o_fin(1)
        out_ref[b] = proj_o(b16(ctxo[0]), b16(ctxo[1])).astype(out_ref.dtype)
        if is_late:
            ret[0].wait_recv()
        y0_r[...] = jnp.dot(b16(ctxr[0]), wo_rows(0), preferred_element_type=f32)
        return nonfinite(ctxs), nonfinite(ctxo), nonfinite(ctxr, (0,))

    bad_s, bad_o, bad_r0 = lax.cond(me == 1, lambda: tail(True), lambda: tail(False))

    @pl.when(bad_s + bad_o > 0)
    def _():
        @pl.when(bad_s > 0)
        def _():
            for p in range(2):
                ctxs2[p] = c32(exact(1, p))
            fix.start()
            fix.wait_send()

        @pl.when(bad_o > 0)
        def _():
            out_ref[b] = proj_o(exact(0, 0), exact(0, 1)).astype(out_ref.dtype)

    ret[1].wait_recv()
    y1 = jnp.dot(b16(ctxr[1]), wo_rows(1), preferred_element_type=f32)
    out_ref[1 - b] = (y0_r[...] + y1).astype(out_ref.dtype)

    @pl.when(bad_r0 + nonfinite(ctxr, (1,)) > 0)
    def _():
        fix.wait_recv()
        out_ref[1 - b] = proj_o(b16(ctxr2[0]), b16(ctxr2[1])).astype(out_ref.dtype)

    swait(ctxs, 3)


def pallas_dist_rope_attn_qseq_b2_sq128_d512_hq4_dh64_kernel(x, Wq, Wk, Wv, Wo):
    XB = (NLD, 4, LR // 2, 128)
    CB = (2, SQ // 2, 128)
    return pl.pallas_call(
        _body,
        out_shape=jax.ShapeDtypeStruct((2, SQ, DM), bf16),
        in_specs=[pl.BlockSpec(memory_space=pl.ANY)] * 6,
        out_specs=pl.BlockSpec(memory_space=pltpu.VMEM),
        scratch_shapes=[
            pltpu.VMEM((2, SQ, DM), f32),
            pltpu.VMEM(XB, i32),
            pltpu.VMEM(XB, i32),
            pltpu.VMEM(XB, i32),
            pltpu.VMEM(XB, i32),
            pltpu.VMEM((3, DM, HD), f32),
            pltpu.VMEM((HD, DM), f32),
            pltpu.VMEM((2, DM // 2, 128), i32),
            pltpu.VMEM((4, DM // 2, 128), i32),
            pltpu.VMEM((4, HD // 2, 128), i32),
            pltpu.VMEM((3, 2, SQ, 128), f32),
            pltpu.VMEM((3, 2, 2, SQ // 2, 128), i32),
            pltpu.VMEM((2, 2, SQ // 2, 128), i32),
            pltpu.VMEM((2, 2, SQ, 128), i32),
            pltpu.VMEM((2, 2, 2 * SQ, 128), f32),
            pltpu.VMEM((2, 2, 2 * SQ, 128), f32),
            pltpu.VMEM(CB, i32),
            pltpu.VMEM(CB, i32),
            pltpu.VMEM((SQ, DM), f32),
            pltpu.VMEM((4, 32, 128), i32),
            pltpu.VMEM((2, 64, 128), f32),
            pltpu.VMEM(CB, i32),
            pltpu.VMEM(CB, i32),
            pltpu.VMEM(CB, i32),
            pltpu.VMEM((4, LR // 2, 128), i32),
            pltpu.VMEM((2, 2, LR // 2, 128), i32),
            pltpu.SemaphoreType.DMA((2 * NLD + 7,)),
            pltpu.SemaphoreType.DMA((7,)),
            pltpu.SemaphoreType.DMA((12,)),
            pltpu.SemaphoreType.REGULAR,
        ],
        compiler_params=pltpu.CompilerParams(
            collective_id=0, vmem_limit_bytes=64 * 1024 * 1024, disable_semaphore_checks=True),
    )(x, Wq, Wk, Wv, Wo, jnp.asarray(_TAB))
```
